```python
import numpy as np

kernel_name = "dist_rmsnorm_colshard_i_m768_n512"

def setup_inputs():
    x = np.random.randn(768, 2048).astype(np.float32)
    gamma = np.random.randn(2048).astype(np.float32)
    return {"x": x, "gamma": gamma}

def reference(x: np.ndarray, gamma: np.ndarray) -> np.ndarray:
    eps = 1e-5
    rms = np.sqrt(np.mean(x * x, axis=1, keepdims=True) + eps)
    return gamma * x / rms
```

```python
import jax
import jax.numpy as jnp
from jax import lax
from jax.experimental import pallas as pl
from jax.experimental.pallas import tpu as pltpu

N_DEV = 4
EPS = 1e-5
LANES = 128
SUBLANES = 8

_A_ROWS = (128, 96, 96)
_B_ROWS = (128, 96, 96, 80, 48)
_B_BIG = 2
_STEPS = (("A0", "B0"), ("A1",), ("B1",), ("A2",), ("B2",), ("B3",), ("B4",))
_DEFER = 2
_SIGNAL_AT = 8
_FINISH = (
    ("a", (0, 1, 2, 3)), ("a", (4, 5)), ("b", 0), ("s", None), ("b", 1),
    ("a", (6, 7)), ("b", 2), ("b", 3), ("b", 4), ("b", 5), ("b", 6), ("b", 7),
)


def _plan(m, n):
    assert sum(_A_ROWS) + sum(_B_ROWS) == m and n % LANES == 0
    info, row = {}, 0
    for tag, sizes in (("A", _A_ROWS), ("B", _B_ROWS)):
        for i, s in enumerate(sizes):
            info["%s%d" % (tag, i)] = (row, s)
            row += s
    names = [nm for step in _STEPS for nm in step]
    cid = {nm: c for c, nm in enumerate(names)}
    chunks = [info[nm] for nm in names]

    def tiles(tag, count, prio):
        out = []
        for i in range(count):
            nm = "%s%d" % (tag, i)
            r0, s = info[nm]
            for r in range(r0, r0 + s, SUBLANES):
                for col in range(0, n, LANES):
                    out.append((cid[nm], r, SUBLANES, col, LANES, prio))
        return out

    n_small_b = len(_B_ROWS) - _B_BIG
    la, lb = tiles("A", len(_A_ROWS), 0), tiles("B", n_small_b, 1)
    descs, i, j = [], 0, 0
    while i < len(la) or j < len(lb):
        if j >= len(lb) or (i < len(la) and i * len(lb) <= j * len(la)):
            descs.append(la[i])
            i += 1
        else:
            descs.append(lb[j])
            j += 1
    for i in range(n_small_b, len(_B_ROWS)):
        r0, s = info["B%d" % i]
        descs.append((cid["B%d" % i], r0, s, 0, n, 1))
    steps = [tuple(cid[nm] for nm in step) for step in _STEPS]
    return chunks, descs, steps


def _diag_mask(groups):
    shape = (groups, SUBLANES, LANES)
    lane = lax.broadcasted_iota(jnp.int32, shape, 2)
    sub = lax.broadcasted_iota(jnp.int32, shape, 1)
    grp = lax.broadcasted_iota(jnp.int32, shape, 0)
    return lane - sub == grp * SUBLANES


def pallas_dist_rmsnorm_colshard_i_m768_n512_kernel(
    x: jax.Array,
    gamma: jax.Array,
):
    m, n = x.shape
    n_global = n * N_DEV
    n_col_tiles = n // LANES
    chunks, descs, steps = _plan(m, n)
    n_chunks = len(chunks)

    def body(x_hbm, g_hbm, o_ref, xbuf, gbuf, comm, dcomm, base,
             in_sems, g_sem, send_sem, recv_sems):
        me = lax.axis_index("i")
        barrier = pltpu.get_barrier_semaphore()

        g_copy = pltpu.make_async_copy(g_hbm, gbuf, g_sem)
        g_copy.start()
        for t, (c, r, rows, col, cols, prio) in enumerate(descs):
            if t == _SIGNAL_AT:
                for k in (2, 1, 3):
                    pl.semaphore_signal(
                        barrier, inc=1, device_id=((me + k) % N_DEV,),
                        device_id_type=pl.DeviceIdType.MESH)
            idx = (pl.ds(r, rows), pl.ds(col, cols))
            pltpu.make_async_copy(
                x_hbm.at[idx], xbuf.at[idx], in_sems.at[c]).start(priority=prio)

        g_copy.wait()
        g = gbuf[...].reshape(1, n) * (float(n_global) ** 0.5)

        rdmas, deferred = {}, []
        for si, step in enumerate(steps):
            for c in step:
                r0, s = chunks[c]
                rows = xbuf.at[pl.ds(r0, s)]
                pltpu.make_async_copy(rows, rows, in_sems.at[c]).wait()
            for c in step:
                r0, s = chunks[c]
                groups = s // SUBLANES
                xc = xbuf[pl.ds(r0, s), :]
                sq = xc * xc
                cols = [sq[:, j * LANES:(j + 1) * LANES] for j in range(n_col_tiles)]
                while len(cols) > 1:
                    cols = [cols[i] + cols[i + 1] if i + 1 < len(cols) else cols[i]
                            for i in range(0, len(cols), 2)]
                rs = jnp.sum(cols[0].reshape(groups, SUBLANES, LANES),
                             axis=2, keepdims=True)
                packed = jnp.sum(jnp.where(_diag_mask(groups), rs, 0.0), axis=0)
                comm[c, 0] = jnp.sum(packed, axis=0, keepdims=True)
            for c in step:
                r0, s = chunks[c]
                o_ref[pl.ds(r0, s), :] = xbuf[pl.ds(r0, s), :] * g
            if si == 0:
                pl.semaphore_wait(barrier, N_DEV - 1)
            for k in (2, 1, 3):
                for c in step:
                    dst = dcomm.at[c] if k == 2 else comm.at[c, (k + 1) // 2]
                    rdma = pltpu.make_async_remote_copy(
                        src_ref=comm.at[c, 0], dst_ref=dst,
                        send_sem=send_sem, recv_sem=recv_sems.at[c * 3 + k - 1],
                        device_id=((me + k) % N_DEV,),
                        device_id_type=pl.DeviceIdType.MESH)
                    rdmas[(c, k)] = rdma
                    if k != 2 and c >= n_chunks - _DEFER:
                        deferred.append(rdma)
                    else:
                        rdma.start()
        for rdma in deferred:
            rdma.start()

        sub = lax.broadcasted_iota(jnp.int32, (SUBLANES, LANES), 0)

        def fold_neighbours(cs):
            for c in cs:
                rdmas[(c, 1)].wait_recv()
                rdmas[(c, 3)].wait_recv()
            for c in cs:
                r0, s = chunks[c]
                groups = s // SUBLANES
                tot = (comm[c, 0] + EPS * n_global) + (comm[c, 1] + comm[c, 2])
                col = jnp.sum(jnp.where(_diag_mask(groups), tot[None], 0.0),
                              axis=2, keepdims=True)
                base[pl.ds(r0, s), :] = jnp.broadcast_to(
                    col, (groups, SUBLANES, LANES)).reshape(s, LANES)

        def finish(c):
            r0, s = chunks[c]
            rdmas[(c, 2)].wait_recv()
            for gi in range(s // SUBLANES):
                rows = pl.ds(r0 + gi * SUBLANES, SUBLANES)
                v = [jnp.full((SUBLANES, LANES), dcomm[c, 0, gi * SUBLANES + q],
                              jnp.float32) for q in range(SUBLANES)]
                for bit in (1, 2, 4):
                    v = [jnp.where((sub & bit) == 0, v[i], v[i + 1])
                         for i in range(0, len(v), 2)]
                inv = lax.rsqrt(base[rows, :] + v[0])
                for j in range(n_col_tiles):
                    cols = pl.ds(j * LANES, LANES)
                    o_ref[rows, cols] = o_ref[rows, cols] * inv

        for kind, arg in _FINISH:
            if kind == "a":
                fold_neighbours(arg)
            elif kind == "b":
                finish(arg)
            else:
                pltpu.make_async_copy(comm, comm, send_sem).wait()

    return pl.pallas_call(
        body,
        out_shape=jax.ShapeDtypeStruct((m, n), x.dtype),
        in_specs=[
            pl.BlockSpec(memory_space=pltpu.MemorySpace.HBM),
            pl.BlockSpec(memory_space=pltpu.MemorySpace.HBM),
        ],
        out_specs=pl.BlockSpec(memory_space=pltpu.MemorySpace.VMEM),
        scratch_shapes=[
            pltpu.VMEM((m, n), jnp.float32),
            pltpu.VMEM((n,), jnp.float32),
            pltpu.VMEM((n_chunks, 3, 1, LANES), jnp.float32),
            pltpu.SMEM((n_chunks, 1, LANES), jnp.float32),
            pltpu.VMEM((m, LANES), jnp.float32),
            pltpu.SemaphoreType.DMA((n_chunks,)),
            pltpu.SemaphoreType.DMA,
            pltpu.SemaphoreType.DMA,
            pltpu.SemaphoreType.DMA((n_chunks * 3,)),
        ],
        compiler_params=pltpu.CompilerParams(
            collective_id=0, disable_semaphore_checks=True),
    )(x, gamma)
```

```python
import jax
import jax.numpy as jnp
from jax import lax
from jax.experimental import pallas as pl
from jax.experimental.pallas import tpu as pltpu

N_DEV = 4
EPS = 1e-5
LANES = 128
SUBLANES = 8

_A_ROWS = (128, 96, 96)
_B_ROWS = (128, 96, 96, 80, 48)
_B_BIG = 2
_STEPS = (("A0", "B0"), ("A1",), ("B1",), ("A2",), ("B2",), ("B3",), ("B4",))
_DEFER = 2
_SIGNAL_AT = 8
_FINISH = (
    ("a", (0, 1, 2, 3)), ("a", (4, 5)), ("b", 0), ("b", 1),
    ("a", (6, 7)), ("b", 2), ("b", 3), ("b", 4), ("b", 5), ("b", 6), ("b", 7),
)


def _plan(m, n):
    assert sum(_A_ROWS) + sum(_B_ROWS) == m and n % LANES == 0
    info, row = {}, 0
    for tag, sizes in (("A", _A_ROWS), ("B", _B_ROWS)):
        for i, s in enumerate(sizes):
            info["%s%d" % (tag, i)] = (row, s)
            row += s
    names = [nm for step in _STEPS for nm in step]
    cid = {nm: c for c, nm in enumerate(names)}
    chunks = [info[nm] for nm in names]

    def tiles(tag, count, prio):
        out = []
        for i in range(count):
            nm = "%s%d" % (tag, i)
            r0, s = info[nm]
            for r in range(r0, r0 + s, SUBLANES):
                for col in range(0, n, LANES):
                    out.append((cid[nm], r, SUBLANES, col, LANES, prio))
        return out

    n_small_b = len(_B_ROWS) - _B_BIG
    la, lb = tiles("A", len(_A_ROWS), 0), tiles("B", n_small_b, 1)
    descs, i, j = [], 0, 0
    while i < len(la) or j < len(lb):
        if j >= len(lb) or (i < len(la) and i * len(lb) <= j * len(la)):
            descs.append(la[i])
            i += 1
        else:
            descs.append(lb[j])
            j += 1
    for i in range(n_small_b, len(_B_ROWS)):
        r0, s = info["B%d" % i]
        descs.append((cid["B%d" % i], r0, s, 0, n, 1))
    steps = [tuple(cid[nm] for nm in step) for step in _STEPS]
    return chunks, descs, steps


def _diag_mask(groups):
    shape = (groups, SUBLANES, LANES)
    lane = lax.broadcasted_iota(jnp.int32, shape, 2)
    sub = lax.broadcasted_iota(jnp.int32, shape, 1)
    grp = lax.broadcasted_iota(jnp.int32, shape, 0)
    return lane - sub == grp * SUBLANES


def pallas_dist_rmsnorm_colshard_i_m768_n512_kernel(
    x: jax.Array,
    gamma: jax.Array,
):
    m, n = x.shape
    n_global = n * N_DEV
    n_col_tiles = n // LANES
    chunks, descs, steps = _plan(m, n)
    n_chunks = len(chunks)

    def body(x_hbm, g_hbm, o_ref, xbuf, gbuf, comm, dcomm, base,
             in_sems, g_sem, send_sems, recv_sems):
        me = lax.axis_index("i")
        barrier = pltpu.get_barrier_semaphore()

        g_copy = pltpu.make_async_copy(g_hbm, gbuf, g_sem)
        g_copy.start()
        for t, (c, r, rows, col, cols, prio) in enumerate(descs):
            if t == _SIGNAL_AT:
                for k in (2, 1, 3):
                    pl.semaphore_signal(
                        barrier, inc=1, device_id=((me + k) % N_DEV,),
                        device_id_type=pl.DeviceIdType.MESH)
            idx = (pl.ds(r, rows), pl.ds(col, cols))
            pltpu.make_async_copy(
                x_hbm.at[idx], xbuf.at[idx], in_sems.at[c]).start(priority=prio)

        g_copy.wait()
        g = gbuf[...].reshape(1, n) * (float(n_global) ** 0.5)

        rdmas, deferred = {}, []
        for si, step in enumerate(steps):
            for c in step:
                r0, s = chunks[c]
                rows = xbuf.at[pl.ds(r0, s)]
                pltpu.make_async_copy(rows, rows, in_sems.at[c]).wait()
            for c in step:
                r0, s = chunks[c]
                groups = s // SUBLANES
                xc = xbuf[pl.ds(r0, s), :]
                sq = xc * xc
                cols = [sq[:, j * LANES:(j + 1) * LANES] for j in range(n_col_tiles)]
                while len(cols) > 1:
                    cols = [cols[i] + cols[i + 1] if i + 1 < len(cols) else cols[i]
                            for i in range(0, len(cols), 2)]
                rs = jnp.sum(cols[0].reshape(groups, SUBLANES, LANES),
                             axis=2, keepdims=True)
                packed = jnp.sum(jnp.where(_diag_mask(groups), rs, 0.0), axis=0)
                comm[c, 0] = jnp.sum(packed, axis=0, keepdims=True)
            for c in step:
                r0, s = chunks[c]
                o_ref[pl.ds(r0, s), :] = xbuf[pl.ds(r0, s), :] * g
            if si == 0:
                pl.semaphore_wait(barrier, N_DEV - 1)
            for k in (2, 1, 3):
                for c in step:
                    dst = dcomm.at[c] if k == 2 else comm.at[c, (k + 1) // 2]
                    rdma = pltpu.make_async_remote_copy(
                        src_ref=comm.at[c, 0], dst_ref=dst,
                        send_sem=send_sems.at[c * 3 + k - 1],
                        recv_sem=recv_sems.at[c * 3 + k - 1],
                        device_id=((me + k) % N_DEV,),
                        device_id_type=pl.DeviceIdType.MESH)
                    rdmas[(c, k)] = rdma
                    if k != 2 and c >= n_chunks - _DEFER:
                        deferred.append(rdma)
                    else:
                        rdma.start()
        for rdma in deferred:
            rdma.start()
        for rdma in rdmas.values():
            rdma.wait_send()

        sub = lax.broadcasted_iota(jnp.int32, (SUBLANES, LANES), 0)

        def fold_neighbours(cs):
            for c in cs:
                rdmas[(c, 1)].wait_recv()
                rdmas[(c, 3)].wait_recv()
            for c in cs:
                r0, s = chunks[c]
                groups = s // SUBLANES
                tot = (comm[c, 0] + EPS * n_global) + (comm[c, 1] + comm[c, 2])
                col = jnp.sum(jnp.where(_diag_mask(groups), tot[None], 0.0),
                              axis=2, keepdims=True)
                base[pl.ds(r0, s), :] = jnp.broadcast_to(
                    col, (groups, SUBLANES, LANES)).reshape(s, LANES)

        def finish(c):
            r0, s = chunks[c]
            rdmas[(c, 2)].wait_recv()
            merged = []
            for gi in range(s // SUBLANES):
                v = [jnp.full((SUBLANES, LANES), dcomm[c, 0, gi * SUBLANES + q],
                              jnp.float32) for q in range(SUBLANES)]
                for bit in (1, 2, 4):
                    v = [jnp.where((sub & bit) == 0, v[i], v[i + 1])
                         for i in range(0, len(v), 2)]
                merged.append(v[0])
            rows = pl.ds(r0, s)
            inv = lax.rsqrt(base[rows, :] + jnp.concatenate(merged, axis=0))
            o_ref[rows, :] = o_ref[rows, :] * jnp.concatenate(
                [inv] * n_col_tiles, axis=1)

        for kind, arg in _FINISH:
            if kind == "a":
                fold_neighbours(arg)
            else:
                finish(arg)

    return pl.pallas_call(
        body,
        out_shape=jax.ShapeDtypeStruct((m, n), x.dtype),
        in_specs=[
            pl.BlockSpec(memory_space=pltpu.MemorySpace.HBM),
            pl.BlockSpec(memory_space=pltpu.MemorySpace.HBM),
        ],
        out_specs=pl.BlockSpec(memory_space=pltpu.MemorySpace.VMEM),
        scratch_shapes=[
            pltpu.VMEM((m, n), jnp.float32),
            pltpu.VMEM((n,), jnp.float32),
            pltpu.VMEM((n_chunks, 3, 1, LANES), jnp.float32),
            pltpu.SMEM((n_chunks, 1, LANES), jnp.float32),
            pltpu.VMEM((m, LANES), jnp.float32),
            pltpu.SemaphoreType.DMA((n_chunks,)),
            pltpu.SemaphoreType.DMA,
            pltpu.SemaphoreType.DMA((n_chunks * 3,)),
            pltpu.SemaphoreType.DMA((n_chunks * 3,)),
        ],
        compiler_params=pltpu.CompilerParams(
            collective_id=0, disable_semaphore_checks=True),
    )(x, gamma)
```
